```python
import numpy as np

kernel_name = "dist_sum_ax1_xy_m512_n256"

def setup_inputs():
    return {"x": np.random.randn(1024, 512).astype(np.float32)}

def reference(x: np.ndarray) -> np.ndarray:
    return np.sum(x, axis=1, keepdims=True)
```

```python
import jax
import jax.numpy as jnp
from jax import lax
from jax.experimental import pallas as pl
from jax.experimental.pallas import tpu as pltpu

_LANES = 128
_SUBLANES = 8


def pallas_dist_sum_ax1_xy_m512_n256_kernel(
x: jax.Array,
):
    m, n = x.shape
    n_groups = m // _LANES
    msgs = ((0, n_groups - 1), (n_groups - 1, n_groups))

    def body(x_hbm, o_ref, xbuf, send_buf, recv_buf, in_sems, send_sems, recv_sems):
        peer = dict(
            device_id=(lax.axis_index("x"), 1 - lax.axis_index("y")),
            device_id_type=pl.DeviceIdType.MESH,
        )

        loads = []
        for g in range(n_groups):
            rows = pl.ds(g * _LANES, _LANES)
            cp = pltpu.make_async_copy(x_hbm.at[rows], xbuf.at[rows], in_sems.at[g])
            cp.start()
            loads.append(cp)

        barrier = pltpu.get_barrier_semaphore()
        pl.semaphore_signal(barrier, inc=1, **peer)

        def msg_cols(k):
            g0, g1 = msgs[k]
            return pl.ds(g0 * _LANES, (g1 - g0) * _LANES)

        rdmas = [
            pltpu.make_async_remote_copy(
                src_ref=send_buf.at[:, msg_cols(k)],
                dst_ref=recv_buf.at[:, msg_cols(k)],
                send_sem=send_sems.at[k],
                recv_sem=recv_sems.at[k],
                **peer,
            )
            for k in range(len(msgs))
        ]

        tile = (_SUBLANES, _LANES)
        lane_minus_sublane = lax.broadcasted_iota(
            jnp.int32, tile, 1
        ) - lax.broadcasted_iota(jnp.int32, tile, 0)

        for g in range(n_groups):
            loads[g].wait()
            acc = None
            for j in range(_LANES // _SUBLANES):
                rows = pl.ds(g * _LANES + j * _SUBLANES, _SUBLANES)
                folded = xbuf[rows, pl.ds(0, _LANES)]
                for c in range(1, n // _LANES):
                    folded = folded + xbuf[rows, pl.ds(c * _LANES, _LANES)]
                row_sum = jnp.sum(folded, axis=1, keepdims=True)
                diag = jnp.where(lane_minus_sublane == j * _SUBLANES, row_sum, 0.0)
                acc = diag if acc is None else acc + diag
            send_buf[:, pl.ds(g * _LANES, _LANES)] = jnp.sum(acc, axis=0, keepdims=True)
            for k, (_, g1) in enumerate(msgs):
                if g1 == g + 1:
                    if k == 0:
                        pl.semaphore_wait(barrier, 1)
                    rdmas[k].start()

        for rdma in rdmas:
            rdma.wait_send()
        for k, rdma in enumerate(rdmas):
            rdma.wait_recv()
            o_ref[:, msg_cols(k)] = send_buf[:, msg_cols(k)] + recv_buf[:, msg_cols(k)]

    out = pl.pallas_call(
        body,
        out_shape=jax.ShapeDtypeStruct((1, m), jnp.float32),
        in_specs=[pl.BlockSpec(memory_space=pl.ANY)],
        out_specs=pl.BlockSpec(memory_space=pltpu.VMEM),
        scratch_shapes=[
            pltpu.VMEM((m, n), jnp.float32),
            pltpu.VMEM((1, m), jnp.float32),
            pltpu.VMEM((1, m), jnp.float32),
            pltpu.SemaphoreType.DMA((n_groups,)),
            pltpu.SemaphoreType.DMA((len(msgs),)),
            pltpu.SemaphoreType.DMA((len(msgs),)),
        ],
        compiler_params=pltpu.CompilerParams(
            collective_id=0, disable_semaphore_checks=True
        ),
    )(x)
    return out.reshape(m, 1)
```

```python
import jax
import jax.numpy as jnp
from jax import lax
from jax.experimental import pallas as pl
from jax.experimental.pallas import tpu as pltpu

_LANES = 128
_SUBLANES = 8
_CHUNK_ROWS = 96
_N_TAIL_CHUNKS = 3


def pallas_dist_sum_ax1_xy_m512_n256_kernel(
x: jax.Array,
):
    m, n = x.shape
    assert m % _LANES == 0 and n % _LANES == 0
    n_groups = m // _LANES
    tiles_per_group = _LANES // _SUBLANES

    bounds = [0] + [m - k * _CHUNK_ROWS for k in range(_N_TAIL_CHUNKS, -1, -1)]
    n_chunks = len(bounds) - 1
    assert bounds[1] > 0
    msgs = ((0, n_groups - 1), (n_groups - 1, n_groups))

    def body(x_hbm, o_ref, xbuf, send_buf, recv_buf, in_sems, send_sems, recv_sems):
        peer = dict(
            device_id=(lax.axis_index("x"), 1 - lax.axis_index("y")),
            device_id_type=pl.DeviceIdType.MESH,
        )

        loads = []
        for c in range(n_chunks):
            rows = pl.ds(bounds[c], bounds[c + 1] - bounds[c])
            load = pltpu.make_async_copy(x_hbm.at[rows], xbuf.at[rows], in_sems.at[c])
            load.start()
            loads.append(load)

        barrier = pltpu.get_barrier_semaphore()
        pl.semaphore_signal(barrier, inc=1, **peer)

        def msg_cols(k):
            g0, g1 = msgs[k]
            return pl.ds(g0 * _LANES, (g1 - g0) * _LANES)

        rdmas = [
            pltpu.make_async_remote_copy(
                src_ref=send_buf.at[:, msg_cols(k)],
                dst_ref=recv_buf.at[:, msg_cols(k)],
                send_sem=send_sems.at[k],
                recv_sem=recv_sems.at[k],
                **peer,
            )
            for k in range(len(msgs))
        ]

        tile = (_SUBLANES, _LANES)
        lane_minus_sublane = lax.broadcasted_iota(
            jnp.int32, tile, 1
        ) - lax.broadcasted_iota(jnp.int32, tile, 0)

        diag = [jnp.zeros(tile, jnp.float32)] * n_groups
        groups_done = 0
        msgs_sent = 0
        for c in range(n_chunks):
            loads[c].wait()
            for r0 in range(bounds[c], bounds[c + 1], _SUBLANES):
                g, j = divmod(r0 // _SUBLANES, tiles_per_group)
                rows = pl.ds(r0, _SUBLANES)
                folded = xbuf[rows, pl.ds(0, _LANES)]
                for k in range(1, n // _LANES):
                    folded = folded + xbuf[rows, pl.ds(k * _LANES, _LANES)]
                row_sum = jnp.sum(folded, axis=1, keepdims=True)
                diag[g] = jnp.where(
                    lane_minus_sublane == j * _SUBLANES, row_sum, diag[g]
                )
            while (groups_done + 1) * _LANES <= bounds[c + 1]:
                send_buf[:, pl.ds(groups_done * _LANES, _LANES)] = jnp.sum(
                    diag[groups_done], axis=0, keepdims=True
                )
                groups_done += 1
            while msgs_sent < len(msgs) and msgs[msgs_sent][1] <= groups_done:
                if msgs_sent == 0:
                    pl.semaphore_wait(barrier, 1)
                rdmas[msgs_sent].start()
                msgs_sent += 1

        for rdma in rdmas:
            rdma.wait_send()
        for k, rdma in enumerate(rdmas):
            rdma.wait_recv()
            o_ref[:, msg_cols(k)] = send_buf[:, msg_cols(k)] + recv_buf[:, msg_cols(k)]

    out = pl.pallas_call(
        body,
        out_shape=jax.ShapeDtypeStruct((1, m), jnp.float32),
        in_specs=[pl.BlockSpec(memory_space=pl.ANY)],
        out_specs=pl.BlockSpec(memory_space=pltpu.VMEM),
        scratch_shapes=[
            pltpu.VMEM((m, n), jnp.float32),
            pltpu.VMEM((1, m), jnp.float32),
            pltpu.VMEM((1, m), jnp.float32),
            pltpu.SemaphoreType.DMA((n_chunks,)),
            pltpu.SemaphoreType.DMA((len(msgs),)),
            pltpu.SemaphoreType.DMA((len(msgs),)),
        ],
        compiler_params=pltpu.CompilerParams(
            collective_id=0,
            disable_semaphore_checks=True,
        ),
    )(x)
    return out.reshape(m, 1)
```

```python
import jax
import jax.numpy as jnp
from jax import lax
from jax.experimental import pallas as pl
from jax.experimental.pallas import tpu as pltpu

_LANES = 128
_SUBLANES = 8
_CHUNK_ROWS = 96
_N_CHUNKS = 3
_EARLY_ROWS = _LANES - _CHUNK_ROWS


def pallas_dist_sum_ax1_xy_m512_n256_kernel(
x: jax.Array,
):
    m, n = x.shape
    assert m % _LANES == 0 and n % _LANES == 0
    n_groups = m // _LANES
    tiles_per_group = _LANES // _SUBLANES

    bulk_end = m - _EARLY_ROWS
    head_rows = bulk_end - _N_CHUNKS * _CHUNK_ROWS
    assert head_rows > 0 and head_rows % _SUBLANES == 0
    stages = [[(bulk_end, _EARLY_ROWS), (0, head_rows)]] + [
        [(head_rows + c * _CHUNK_ROWS, _CHUNK_ROWS)] for c in range(_N_CHUNKS)
    ]
    n_loads = sum(len(stage) for stage in stages)
    msgs = ((0, n_groups - 1), (n_groups - 1, n_groups))

    def body(x_hbm, o_ref, xbuf, send_buf, recv_buf, in_sems, send_sems, recv_sems):
        peer = dict(
            device_id=(lax.axis_index("x"), 1 - lax.axis_index("y")),
            device_id_type=pl.DeviceIdType.MESH,
        )

        loads = {}
        for stage in stages:
            for start, size in stage:
                rows = pl.ds(start, size)
                load = pltpu.make_async_copy(
                    x_hbm.at[rows], xbuf.at[rows], in_sems.at[len(loads)]
                )
                load.start()
                loads[start] = load

        barrier = pltpu.get_barrier_semaphore()
        pl.semaphore_signal(barrier, inc=1, **peer)

        def msg_cols(k):
            g0, g1 = msgs[k]
            return pl.ds(g0 * _LANES, (g1 - g0) * _LANES)

        rdmas = [
            pltpu.make_async_remote_copy(
                src_ref=send_buf.at[:, msg_cols(k)],
                dst_ref=recv_buf.at[:, msg_cols(k)],
                send_sem=send_sems.at[k],
                recv_sem=recv_sems.at[k],
                **peer,
            )
            for k in range(len(msgs))
        ]

        tile = (_SUBLANES, _LANES)
        lane_minus_sublane = lax.broadcasted_iota(
            jnp.int32, tile, 1
        ) - lax.broadcasted_iota(jnp.int32, tile, 0)

        diag = [jnp.zeros(tile, jnp.float32)] * n_groups
        tiles_left = [tiles_per_group] * n_groups
        msgs_sent = 0
        for stage in stages:
            for start, _ in stage:
                loads[start].wait()
            finished = []
            for start, size in stage:
                for r0 in range(start, start + size, _SUBLANES):
                    g, j = divmod(r0 // _SUBLANES, tiles_per_group)
                    rows = pl.ds(r0, _SUBLANES)
                    folded = xbuf[rows, pl.ds(0, _LANES)]
                    for k in range(1, n // _LANES):
                        folded = folded + xbuf[rows, pl.ds(k * _LANES, _LANES)]
                    row_sum = jnp.sum(folded, axis=1, keepdims=True)
                    diag[g] = jnp.where(
                        lane_minus_sublane == j * _SUBLANES, row_sum, diag[g]
                    )
                    tiles_left[g] -= 1
                    if tiles_left[g] == 0:
                        finished.append(g)
            for g in finished:
                send_buf[:, pl.ds(g * _LANES, _LANES)] = jnp.sum(
                    diag[g], axis=0, keepdims=True
                )
            while msgs_sent < len(msgs) and not any(
                tiles_left[slice(*msgs[msgs_sent])]
            ):
                if msgs_sent == 0:
                    pl.semaphore_wait(barrier, 1)
                rdmas[msgs_sent].start()
                msgs_sent += 1
        assert msgs_sent == len(msgs)

        for rdma in rdmas:
            rdma.wait_send()
        for k, rdma in enumerate(rdmas):
            rdma.wait_recv()
            o_ref[:, msg_cols(k)] = send_buf[:, msg_cols(k)] + recv_buf[:, msg_cols(k)]

    out = pl.pallas_call(
        body,
        out_shape=jax.ShapeDtypeStruct((1, m), jnp.float32),
        in_specs=[pl.BlockSpec(memory_space=pl.ANY)],
        out_specs=pl.BlockSpec(memory_space=pltpu.VMEM),
        scratch_shapes=[
            pltpu.VMEM((m, n), jnp.float32),
            pltpu.VMEM((1, m), jnp.float32),
            pltpu.VMEM((1, m), jnp.float32),
            pltpu.SemaphoreType.DMA((n_loads,)),
            pltpu.SemaphoreType.DMA((len(msgs),)),
            pltpu.SemaphoreType.DMA((len(msgs),)),
        ],
        compiler_params=pltpu.CompilerParams(
            collective_id=0,
            disable_semaphore_checks=True,
        ),
    )(x)
    return out.reshape(m, 1)
```
